```python
import numpy as np

kernel_name = "dist_layernorm_xy_m6144_n2048"

def setup_inputs():
    x = np.random.randn(12288, 4096).astype(np.float32)
    gamma = np.random.randn(4096).astype(np.float32)
    beta = np.random.randn(4096).astype(np.float32)
    return {"x": x, "gamma": gamma, "beta": beta}

def reference(x: np.ndarray, gamma: np.ndarray, beta: np.ndarray) -> np.ndarray:
    eps = 1e-5
    mean = np.mean(x, axis=1, keepdims=True)
    var = np.var(x, axis=1, keepdims=True)
    return gamma * (x - mean) / np.sqrt(var + eps) + beta
```

```python
import jax
import jax.numpy as jnp
from jax import lax
from jax.experimental import pallas as pl
from jax.experimental.pallas import tpu as pltpu

EPS = 1e-5
LANES = 128
N_Y = 2
CH = 256
RB = 64
LAG = 1


def pallas_dist_layernorm_xy_m6144_n2048_kernel(
    x: jax.Array,
    gamma: jax.Array,
    beta: jax.Array,
):
    m, n = x.shape
    assert m % CH == 0 and CH % RB == 0 and n % LANES == 0
    nch = m // CH
    ntile = n // LANES
    n_total = n * N_Y

    def body(x_hbm, g_ref, b_ref, o_ref,
             stat_a, stat_b, sbuf, rbuf,
             in_sems, send_sems, recv_sems):
        my_x = lax.axis_index("x")
        my_y = lax.axis_index("y")
        peer = (my_x, 1 - my_y)

        def in_copy(c):
            return pltpu.make_async_copy(
                x_hbm.at[pl.ds(c * CH, CH)], o_ref.at[pl.ds(c * CH, CH)], in_sems.at[c])

        def stats_rdma(c):
            return pltpu.make_async_remote_copy(
                src_ref=sbuf.at[:, pl.ds(c * CH, CH)], dst_ref=rbuf.at[:, pl.ds(c * CH, CH)],
                send_sem=send_sems.at[c], recv_sem=recv_sems.at[c],
                device_id=peer, device_id_type=pl.DeviceIdType.MESH)

        for c in range(nch):
            in_copy(c).start()

        barrier_sem = pltpu.get_barrier_semaphore()
        pl.semaphore_signal(barrier_sem, inc=1, device_id=peer,
                            device_id_type=pl.DeviceIdType.MESH)
        pl.semaphore_wait(barrier_sem, 1)

        def local_stats(c):
            base = c * CH

            def blk(i, carry):
                r0 = pl.multiple_of(i * RB, RB)
                rows = pl.ds(base + r0, RB)
                p1 = o_ref[rows, 0:LANES]
                for j in range(1, ntile):
                    p1 = p1 + o_ref[rows, j * LANES:(j + 1) * LANES]
                mean = jnp.sum(p1, axis=1, keepdims=True) * (1.0 / n)
                p2 = None
                for j in range(ntile):
                    d = o_ref[rows, j * LANES:(j + 1) * LANES] - mean
                    p2 = d * d if p2 is None else p2 + d * d
                stat_a[pl.ds(r0, RB), :] = jnp.broadcast_to(mean, (RB, LANES))
                stat_b[pl.ds(r0, RB), :] = p2
                return carry

            lax.fori_loop(0, CH // RB, blk, 0)
            mean_t = stat_a[...].T
            m2_row = jnp.sum(stat_b[...].T, axis=0, keepdims=True)
            cols = pl.ds(base, CH)
            sbuf[0:1, cols] = mean_t[0:1, :]
            sbuf[1:2, cols] = m2_row
            sbuf[2:8, cols] = jnp.zeros((6, CH), jnp.float32)

        def finish(c):
            base = c * CH
            cols = pl.ds(base, CH)
            mean_l = sbuf[0:1, cols]
            m2_l = sbuf[1:2, cols]
            mean_r = rbuf[0:1, cols]
            m2_r = rbuf[1:2, cols]
            mean = (mean_l + mean_r) * 0.5
            delta = mean_r - mean_l
            m2 = (m2_l + m2_r) + (delta * delta) * (n * 0.5)
            var = m2 * (1.0 / n_total)
            rstd = lax.rsqrt(var + EPS)
            stat_a[...] = jnp.broadcast_to(mean, (LANES, CH)).T
            stat_b[...] = jnp.broadcast_to(rstd, (LANES, CH)).T

            def blk(i, carry):
                r0 = pl.multiple_of(i * RB, RB)
                rows = pl.ds(base + r0, RB)
                mu = stat_a[pl.ds(r0, RB), :]
                rs = stat_b[pl.ds(r0, RB), :]
                for j in range(ntile):
                    cs = slice(j * LANES, (j + 1) * LANES)
                    xj = o_ref[rows, cs]
                    o_ref[rows, cs] = (xj - mu) * rs * g_ref[:, cs] + b_ref[:, cs]
                return carry

            lax.fori_loop(0, CH // RB, blk, 0)

        for c in range(nch):
            in_copy(c).wait()
            local_stats(c)
            stats_rdma(c).start()
            if c >= LAG:
                d = c - LAG
                stats_rdma(d).wait_recv()
                finish(d)
        for d in range(nch - LAG, nch):
            stats_rdma(d).wait_recv()
            finish(d)
        for c in range(nch):
            stats_rdma(c).wait_send()

    return pl.pallas_call(
        body,
        out_shape=pltpu.VMEM((m, n), x.dtype),
        in_specs=[pl.BlockSpec(memory_space=pl.ANY),
                  pl.BlockSpec(memory_space=pltpu.VMEM),
                  pl.BlockSpec(memory_space=pltpu.VMEM)],
        out_specs=pl.BlockSpec(memory_space=pltpu.VMEM),
        scratch_shapes=[
            pltpu.VMEM((CH, LANES), jnp.float32),
            pltpu.VMEM((CH, LANES), jnp.float32),
            pltpu.VMEM((8, m), jnp.float32),
            pltpu.VMEM((8, m), jnp.float32),
            pltpu.SemaphoreType.DMA((nch,)),
            pltpu.SemaphoreType.DMA((nch,)),
            pltpu.SemaphoreType.DMA((nch,)),
        ],
        compiler_params=pltpu.CompilerParams(
            collective_id=0, vmem_limit_bytes=32 * 1024 * 1024),
    )(x, gamma.reshape(1, n), beta.reshape(1, n))
```

```python
import jax
import jax.numpy as jnp
from jax import lax
from jax.experimental import pallas as pl
from jax.experimental.pallas import tpu as pltpu

EPS = 1e-5
LANES = 128
N_Y = 2
MAX_CH = 256
TAIL = (128, 64, 64)
RBF = 64


def _compiler_params():
    kwargs = dict(collective_id=0, vmem_limit_bytes=32 * 1024 * 1024)
    try:
        return pltpu.CompilerParams(**kwargs, disable_semaphore_checks=True)
    except TypeError:
        return pltpu.CompilerParams(**kwargs)


def pallas_dist_layernorm_xy_m6144_n2048_kernel(
    x: jax.Array,
    gamma: jax.Array,
    beta: jax.Array,
):
    m, n = x.shape
    assert n % LANES == 0 and m % MAX_CH == 0 and sum(TAIL) == MAX_CH
    n_full = m // MAX_CH - 1
    tail = []
    row = n_full * MAX_CH
    for k, size in enumerate(TAIL):
        assert size % 8 == 0 and size % min(RBF, size) == 0
        tail.append((n_full + k, row, size))
        row += size
    nch = n_full + len(TAIL)
    ntile = n // LANES
    n_total = n * N_Y

    def body(x_hbm, g_hbm, b_hbm, o_ref,
             gbuf, bbuf, stat_a, stat_b, sbuf, rbuf,
             in_sems, gb_sems, send_sems, recv_sems):
        my_x = lax.axis_index("x")
        my_y = lax.axis_index("y")
        peer = (my_x, 1 - my_y)

        def in_copy(slot, start, size):
            return pltpu.make_async_copy(
                x_hbm.at[pl.ds(start, size)], o_ref.at[pl.ds(start, size)], in_sems.at[slot])

        def stats_rdma(slot):
            width = MAX_CH
            if isinstance(slot, int) and slot >= n_full:
                width = -(-TAIL[slot - n_full] // LANES) * LANES
            return pltpu.make_async_remote_copy(
                src_ref=sbuf.at[slot, :, pl.ds(0, width)],
                dst_ref=rbuf.at[slot, :, pl.ds(0, width)],
                send_sem=send_sems.at[slot], recv_sem=recv_sems.at[slot],
                device_id=peer, device_id_type=pl.DeviceIdType.MESH)

        g_copy = pltpu.make_async_copy(g_hbm, gbuf, gb_sems.at[0])
        b_copy = pltpu.make_async_copy(b_hbm, bbuf, gb_sems.at[1])

        g_copy.start()
        b_copy.start()
        in_copy(0, 0, MAX_CH).start()
        g_copy.wait()
        b_copy.wait()
        for c in range(1, n_full):
            in_copy(c, c * MAX_CH, MAX_CH).start()
        for slot, start, size in tail:
            in_copy(slot, start, size).start()

        barrier_sem = pltpu.get_barrier_semaphore()
        pl.semaphore_signal(barrier_sem, inc=1, device_id=peer,
                            device_id_type=pl.DeviceIdType.MESH)
        pl.semaphore_wait(barrier_sem, 1)

        row_id = lax.broadcasted_iota(jnp.int32, (LANES, LANES), 0)
        lane_id = lax.broadcasted_iota(jnp.int32, (LANES, LANES), 1)
        eye = row_id == lane_id

        def local_stats(slot, start, size):
            rows = pl.ds(start, size)
            p1 = o_ref[rows, 0:LANES]
            for j in range(1, ntile):
                p1 = p1 + o_ref[rows, j * LANES:(j + 1) * LANES]
            mean = jnp.sum(p1, axis=1, keepdims=True) * (1.0 / n)
            stat_a[0:size, :] = jnp.broadcast_to(mean, (size, LANES))
            mu = stat_a[0:size, :]
            p2 = None
            for j in range(ntile):
                d = o_ref[rows, j * LANES:(j + 1) * LANES] - mu
                p2 = d * d if p2 is None else p2 + d * d
            m2 = jnp.sum(p2, axis=1, keepdims=True)
            stat_b[0:size, :] = jnp.broadcast_to(m2, (size, LANES))
            for b0 in range(0, size, LANES):
                cols = slice(b0, b0 + LANES)
                valid = min(size - b0, LANES)
                mask = eye if valid == LANES else jnp.logical_and(eye, row_id < valid)
                sa = stat_a[b0:b0 + LANES, :]
                sb = stat_b[b0:b0 + LANES, :]
                sbuf[slot, 0:1, cols] = jnp.sum(jnp.where(mask, sa, 0.0), axis=0, keepdims=True)
                sbuf[slot, 1:2, cols] = jnp.sum(jnp.where(mask, sb, 0.0), axis=0, keepdims=True)
                sbuf[slot, 2:8, cols] = jnp.zeros((6, LANES), jnp.float32)

        def finish(slot, start, size):
            for b0 in range(0, size, LANES):
                cols = slice(b0, b0 + LANES)
                mean_l = sbuf[slot, 0:1, cols]
                m2_l = sbuf[slot, 1:2, cols]
                mean_r = rbuf[slot, 0:1, cols]
                m2_r = rbuf[slot, 1:2, cols]
                mean = (mean_l + mean_r) * 0.5
                delta = mean_r - mean_l
                m2 = (m2_l + m2_r) + (delta * delta) * (n * 0.5)
                var = m2 * (1.0 / n_total)
                rstd = lax.rsqrt(var + EPS)
                mb = jnp.broadcast_to(mean, (LANES, LANES))
                rb = jnp.broadcast_to(rstd, (LANES, LANES))
                mcol = jnp.sum(jnp.where(eye, mb, 0.0), axis=1, keepdims=True)
                rcol = jnp.sum(jnp.where(eye, rb, 0.0), axis=1, keepdims=True)
                stat_a[b0:b0 + LANES, :] = jnp.broadcast_to(mcol, (LANES, LANES))
                stat_b[b0:b0 + LANES, :] = jnp.broadcast_to(rcol, (LANES, LANES))
            rb_rows = min(RBF, size)
            for r0 in range(0, size, rb_rows):
                rows = pl.ds(start + r0, rb_rows)
                mu = stat_a[r0:r0 + rb_rows, :]
                rs = stat_b[r0:r0 + rb_rows, :]
                for j in range(ntile):
                    cs = slice(j * LANES, (j + 1) * LANES)
                    xj = o_ref[rows, cs]
                    o_ref[rows, cs] = (xj - mu) * rs * gbuf[:, cs] + bbuf[:, cs]

        in_copy(0, 0, MAX_CH).wait()
        local_stats(0, 0, MAX_CH)
        stats_rdma(0).start()

        def step(c, carry):
            start = pl.multiple_of(c * MAX_CH, MAX_CH)
            prev = pl.multiple_of((c - 1) * MAX_CH, MAX_CH)
            in_copy(c, start, MAX_CH).wait()
            local_stats(c, start, MAX_CH)
            stats_rdma(c).start()
            stats_rdma(c - 1).wait_recv()
            finish(c - 1, prev, MAX_CH)
            return carry

        lax.fori_loop(1, n_full, step, 0)

        for slot, start, size in tail:
            in_copy(slot, start, size).wait()
            local_stats(slot, start, size)
            stats_rdma(slot).start()
        for slot, start, size in [(n_full - 1, (n_full - 1) * MAX_CH, MAX_CH)] + tail:
            stats_rdma(slot).wait_recv()
            finish(slot, start, size)

        def drain(c, carry):
            stats_rdma(c).wait_send()
            return carry

        lax.fori_loop(0, n_full, drain, 0)
        for slot, _, _ in tail:
            stats_rdma(slot).wait_send()

    return pl.pallas_call(
        body,
        out_shape=pltpu.VMEM((m, n), x.dtype),
        in_specs=[pl.BlockSpec(memory_space=pl.ANY)] * 3,
        out_specs=pl.BlockSpec(memory_space=pltpu.VMEM),
        scratch_shapes=[
            pltpu.VMEM((1, n), jnp.float32),
            pltpu.VMEM((1, n), jnp.float32),
            pltpu.VMEM((MAX_CH, LANES), jnp.float32),
            pltpu.VMEM((MAX_CH, LANES), jnp.float32),
            pltpu.VMEM((nch, 8, MAX_CH), jnp.float32),
            pltpu.VMEM((nch, 8, MAX_CH), jnp.float32),
            pltpu.SemaphoreType.DMA((nch,)),
            pltpu.SemaphoreType.DMA((2,)),
            pltpu.SemaphoreType.DMA((nch,)),
            pltpu.SemaphoreType.DMA((nch,)),
        ],
        compiler_params=_compiler_params(),
    )(x, gamma.reshape(1, n), beta.reshape(1, n))
```
